```python
import numpy as np

kernel_name = "dist_ag_xy_y_m65536_n1024"

def setup_inputs():
    return {"x": np.random.randn(131072, 1024).astype(np.float32)}

def reference(x: np.ndarray) -> np.ndarray:
    return x
```

```python
import jax
import jax.numpy as jnp
from jax import lax
from jax.experimental import pallas as pl
from jax.experimental.pallas import tpu as pltpu

PIECE_ROWS = 16
PIECES = 64
KEPT = 28
KEPT_SHIFT = 17

RUNS = 8
LANES = 512
GROUPS = 8

RATE_NUM = 429
RATE_SHIFT = 8
WINDOW = 8
AHEAD = 4
RING = 16
MAX_WORDS = 4
FIRST_BASE = 127
RAW_TAG = 0x5A3C97

LOW_AT = 0
ODD_AT = LOW_AT + 8 * GROUPS
WORDS_AT = ODD_AT + 8
HIGH_AT = WORDS_AT + 8 * MAX_WORDS
PACKET_ROWS = HIGH_AT + 8 * GROUPS
TAIL_AT = 48

SEND_SLOTS = AHEAD + 3
Y_SLOTS = 8
X_SLOTS = 8
CREDIT = 4
Y_LAG = 2
X_LAG = 4
PRIVATE_LAG = 3
LOAD_SLOTS = 3
STORE_SLOTS = 2

assert 1 << RATE_SHIFT <= RATE_NUM <= 2 << RATE_SHIFT
assert (AHEAD + 1) * RATE_NUM >> RATE_SHIFT >= WINDOW
assert max(WINDOW + 2, 2 * (AHEAD + 2)) <= RING
assert Y_SLOTS > CREDIT + Y_LAG and X_SLOTS + Y_LAG > max(CREDIT, AHEAD) + X_LAG
assert 1 <= PRIVATE_LAG <= X_LAG


def _bytes(b):
    v = b * 0x01010101
    return v - (1 << 32) if v >= 1 << 31 else v


def _shl(v, n):
    return lax.shift_left(v, jnp.int32(n) if isinstance(n, int) else n)


def _shr(v, n):
    return lax.shift_right_logical(v, jnp.int32(n) if isinstance(n, int) else n)


def _rotl(v, n):
    return _shl(v, n) | _shr(v, 32 - n)


def _at_least(v, n):
    return _shr(v + _bytes(128 - n), 7) & _bytes(1)


def _at_most(v, n):
    return _shr(_bytes(128 + n) - v, 7) & _bytes(1)


def _replace(v, where, new):
    return v ^ ((v ^ new) & (where - _shr(where, 7)))


def _subtract_from(base):
    c = ((base + 2) & 0xFF) * 0x01010101
    top = _bytes(0x80)
    unborrowed = jnp.full((8, LANES), c | top, jnp.int32)
    flipped = jnp.full((8, LANES), ~c, jnp.int32)
    return lambda v: (unborrowed - (v & ~top)) ^ ((flipped ^ v) & top)


def _split(a, b):
    b = _rotl(b, 8)
    t = (a ^ b) & 0x7F807F80
    return a ^ t, _rotl(b ^ t, 1)


def _join(low, high):
    high = _rotl(high, 31)
    t = (low ^ high) & 0x7F807F80
    return low ^ t, _rotl(high ^ t, 24)


def _rank(u):
    rank = u + _at_least(u, 7) + _at_least(u, 14) + _bytes(128 - 2)
    small = (_bytes(128 + 1) - u) & _bytes(0x80)
    return _replace(rank, small, _shl(u & _bytes(1), 3) ^ _bytes(13))


def _unrank(rank):
    u = rank + _at_most(rank, 4) + _at_most(rank, 12)
    moved = (_bytes(0x80) - ((rank & _bytes(0x77)) ^ _bytes(5))) & _bytes(0x80)
    return _replace(u, moved, _shr(~rank, 3) & _bytes(1))


def _floor(t):
    return (t * RATE_NUM) >> RATE_SHIFT


def _blocks_encoded(s):
    return jnp.clip(2 * s + 1, 0, s + 1 + AHEAD)


def _words_sent(s):
    return _floor(_blocks_encoded(s))


def _blocks_decodable(s):
    return jnp.maximum(_blocks_encoded(s) - AHEAD, 0)


def _rebase(pos, t):
    return jnp.maximum(pos - 32 * (_floor(t + 1) - _floor(t)), 0)


def _word(ring, i):
    return ring.at[pl.ds(pl.multiple_of((i & (RING - 1)) * 8, 8), 8)]


def _slab(packet, at, k=0):
    return packet.at[pl.ds(at + 8 * k, 8)]


def _group_place(k):
    across = 1024 // LANES
    run = 2 * (k // across)
    return (run, run + 1), pl.ds(LANES * (k % across), LANES)


def _encode(t, src, dst, packet, ring, pos, pend, base):
    subtract = _subtract_from(base)
    window = [_word(ring, _floor(t) + i) for i in range(WINDOW)]
    odds = seen = longest = None
    for k in range(GROUPS):
        runs, cols = _group_place(k)
        pair = []
        for r in runs:
            rounded = src[r, :, cols].astype(jnp.bfloat16)
            dst[r, :, cols] = rounded
            pair.append(pltpu.bitcast(rounded, jnp.int32))
        low, high = _split(*pair)
        _slab(packet, LOW_AT, k)[...] = low
        _slab(packet, HIGH_AT, k)[...] = high

        u = subtract(high)
        rank = _rank(u)
        odd = rank & _bytes(1)
        z0, z1, z2, z3 = (_shr(rank, 8 * i + 1) & 31 for i in range(4))
        code = _shl(jnp.full_like(z1, 2), z1) | 1
        code = _shl(code + code, z2) | 1
        code = _shl(code + code, z3) | 1
        bits = (z0 + z1) + (z2 + z3 + 4)
        seen = u if k == 0 else seen | u
        odds = odd if k == 0 else odds | _shl(odd, k)
        longest = bits if k == 0 else jnp.maximum(longest, bits)

        top = _shl(code, -bits & 31)
        used = pos & 31
        word = pend | _shr(top, used)
        rest = _shl(_shl(top, 1), used ^ 31)
        at = _shr(pos, 5)
        for i in range(WINDOW):
            pltpu.store(window[i], word, mask=at == i)
        pos = pos + bits
        pend = jnp.where(_shr(pos, 5) != at, rest, word)

    _slab(packet, ODD_AT)[...] = odds
    unfit = ((seen & _bytes(0xC0)) != 0) | (longest > 32) | (pos > 32 * WINDOW)
    unfit = unfit | (_shr(odds, 8) == RAW_TAG)
    return pos, pend, jnp.max(unfit.astype(jnp.int32))


def _put_group(k, low, high, dst):
    runs, cols = _group_place(k)
    for r, words in zip(runs, _join(low, high)):
        dst[r, :, cols] = pltpu.bitcast(words, jnp.bfloat16)


def _decode(t, packet, ring, pos, base, dst):
    subtract = _subtract_from(base)
    window = [_word(ring, _floor(t) + i) for i in range(WINDOW)]

    def gather(refs, at):
        words = [ref[...] for ref in refs]
        bit = 1
        while len(words) > 1:
            upper = (at & bit) != 0
            words = [
                jnp.where(upper, words[i + 1], words[i]) if i + 1 < len(words) else words[i]
                for i in range(0, len(words), 2)
            ]
            bit *= 2
        return words[0]

    odds = _slab(packet, ODD_AT)[...]
    at = _shr(pos, 5)
    cur = gather(window, at)
    for k in range(GROUPS):
        nxt = gather(window[1:], at)
        used = pos & 31
        w = _shl(cur, used) | _shr(_shr(nxt, 1), used ^ 31)
        z0 = lax.clz(w)
        w = _shl(_shl(w, z0), 1)
        z1 = lax.clz(w)
        w = _shl(_shl(w, z1), 1)
        z2 = lax.clz(w)
        w = _shl(_shl(w, z2), 1)
        z3 = lax.clz(w)
        pos = pos + ((z0 + z1) + (z2 + z3 + 4))
        was, at = at, _shr(pos, 5)
        cur = jnp.where(at != was, nxt, cur)

        zeros = (z0 | _shl(z1, 8)) | (_shl(z2, 16) | _shl(z3, 24))
        rank = (zeros + zeros) | (_shr(odds, k) & _bytes(1))
        _put_group(k, _slab(packet, LOW_AT, k)[...], subtract(_unrank(rank)), dst)
    return pos


def _kernel(
    x_hbm,
    kept,
    spilled,
    loaded,
    rounded,
    outbox,
    y_inbox,
    x_inbox,
    rings,
    state,
    bases,
    sent_raw,
    y_raw,
    x_raw,
    load_sem,
    store_sem,
    send_sem,
    relay_sem,
    y_sem,
    x_sem,
    y_credit,
    x_credit,
):
    runs_per_half = x_hbm.shape[0] // 2
    blocks = runs_per_half // RUNS * PIECES
    mx, my = lax.axis_index("x"), lax.axis_index("y")
    y_peer, x_peer = (mx, 1 - my), (1 - mx, my)
    mesh_id = pl.DeviceIdType.MESH

    SHARED, FROM_Y, FROM_X, PRIVATE = range(4)
    quarter = {
        SHARED: 2 * my + mx,
        PRIVATE: 2 * my + 1 - mx,
        FROM_Y: 2 * (1 - my) + mx,
        FROM_X: 2 * (1 - my) + 1 - mx,
    }

    def start(copy):
        copy.start()

    def done(copy):
        copy.wait()

    def sent(copy):
        copy.wait_send()

    def arrived(copy):
        copy.wait_recv()

    def piece_of(t):
        return PIECES - 1 - t % PIECES

    def piece_rows(piece):
        return pl.ds(pl.multiple_of(piece * PIECE_ROWS, PIECE_ROWS), PIECE_ROWS)

    def load(side, t):
        half = mx if side == SHARED else 1 - mx
        runs = pl.ds(half * runs_per_half + t // PIECES * RUNS, RUNS)
        slot = (side == PRIVATE) * LOAD_SLOTS + t % LOAD_SLOTS
        src = x_hbm.at[runs, piece_rows(piece_of(t))]
        return pltpu.make_async_copy(src, loaded.at[slot], load_sem.at[slot]), loaded.at[slot]

    def staging(side, t):
        return rounded.at[side * STORE_SLOTS + t % STORE_SLOTS]

    def store(side, t, act):
        piece = piece_of(t)
        runs = pl.ds(quarter[side] * runs_per_half + t // PIECES * RUNS, RUNS)
        sem = store_sem.at[side * STORE_SLOTS + t % STORE_SLOTS]

        @pl.when(piece < KEPT)
        def _():
            dst = kept.at[runs, piece_rows((piece + KEPT_SHIFT) % KEPT)]
            act(pltpu.make_async_copy(staging(side, t), dst, sem))

        @pl.when(piece >= KEPT)
        def _():
            dst = spilled.at[runs, piece_rows(piece - KEPT)]
            act(pltpu.make_async_copy(staging(side, t), dst, sem))

    def free_staging(side, t):
        @pl.when(t >= STORE_SLOTS)
        def _():
            store(side, t - STORE_SLOTS, done)

    def hop(src, src_slots, src_sem, dst, dst_slots, dst_sem, peer):
        def copy(s, part, rows):
            i, j = s % src_slots, s % dst_slots
            return pltpu.make_async_remote_copy(
                src.at[i, rows],
                dst.at[j, rows],
                src_sem.at[3 * i + part],
                dst_sem.at[3 * j + part],
                device_id=peer,
                device_id_type=mesh_id,
            )

        def head(s, act):
            act(copy(s, 0, pl.ds(0, TAIL_AT)))

        def tail(s, act):
            words = _words_sent(s) - _words_sent(s - 1)
            for n in range(1, MAX_WORDS + 1):

                @pl.when(words == n)
                def _(n=n):
                    act(copy(s, 1, pl.ds(TAIL_AT, WORDS_AT + 8 * n - TAIL_AT)))

        def extra(s, raw, act):
            @pl.when(raw != 0)
            def _():
                act(copy(s, 2, pl.ds(HIGH_AT, 8 * GROUPS)))

        return head, tail, extra

    def whole(link, s, raw, act):
        head, tail, extra = link
        head(s, act)
        tail(s, act)
        extra(s, raw, act)

    y_hop = hop(outbox, SEND_SLOTS, send_sem, y_inbox, Y_SLOTS, y_sem, y_peer)
    x_hop = hop(y_inbox, Y_SLOTS, relay_sem, x_inbox, X_SLOTS, x_sem, x_peer)
    (y_head, y_tail, y_extra), (x_head, x_tail, x_extra) = y_hop, x_hop

    def give_credit(t, slots, credit, peer):
        @pl.when((t % CREDIT == CREDIT - 1) & (t - (CREDIT - 1) + slots < blocks))
        def _():
            sem = credit.at[t // CREDIT % 2]
            pl.semaphore_signal(sem, 1, device_id=peer, device_id_type=mesh_id)

    def take_credit(t, slots, credit):
        @pl.when((t >= slots) & ((t - slots) % CREDIT == 0))
        def _():
            pl.semaphore_wait(credit.at[(t - slots) // CREDIT % 2], 1)

    def for_words(s, move):
        first = _words_sent(s - 1)

        @pl.loop(0, _words_sent(s) - first)
        def _(i):
            move(pl.ds(pl.multiple_of(WORDS_AT + 8 * i, 8), 8), first + i)

    def encode(t):
        ring, pos_ref, pend_ref = rings.at[SHARED], state.at[SHARED], state.at[3]
        packet = outbox.at[t % SEND_SLOTS]

        @pl.when(t >= SEND_SLOTS)
        def _():
            whole(y_hop, t - SEND_SLOTS, sent_raw[t % SEND_SLOTS], sent)

        free_staging(SHARED, t)
        copy, src = load(SHARED, t)
        copy.wait()

        @pl.when(t == 0)
        def _():
            for later in range(1, LOAD_SLOTS):
                load(SHARED, later)[0].start()

        pos, pend, raw = _encode(
            t, src, staging(SHARED, t), packet, ring, pos_ref[...], pend_ref[...], bases[SHARED]
        )
        store(SHARED, t, start)
        sent_raw[t % SEND_SLOTS] = raw

        @pl.when(t + LOAD_SLOTS < blocks)
        def _():
            load(SHARED, t + LOAD_SLOTS)[0].start()

        @pl.when(raw == 0)
        def _():
            pos_ref[...] = pos
            pend_ref[...] = pend

        @pl.when(raw != 0)
        def _():
            high = packet[pl.ds(HIGH_AT, 8 * GROUPS)]
            sixteenths = jnp.sum(high & 0xFF) * 16 // high.size
            base = ((sixteenths + 30) >> 4) & 0xFF
            bases[SHARED] = base
            _slab(packet, ODD_AT)[...] = jnp.full((8, LANES), RAW_TAG << 8 | base, jnp.int32)

        pos, pend = pos_ref[...], pend_ref[...]
        at = _shr(pos, 5)
        for i in range(2):
            pltpu.store(_word(ring, _floor(t) + i), pend, mask=at == i)

        @pl.when(t == blocks - 1)
        def _():
            for i in range(2, WINDOW):
                pltpu.store(_word(ring, _floor(t) + i), pend, mask=at == i)

        pos_ref[...] = _rebase(pos, t)
        pend_ref[...] = jnp.where(at < _floor(t + 1) - _floor(t), 0, pend)

    def receive_tail(s, inbox, slots, flags, tail, extra):
        tail(s, arrived)
        tag = inbox[s % slots, pl.ds(ODD_AT, 8), pl.ds(0, 128)][0, 0]
        raw = jnp.where(_shr(tag, 8) == RAW_TAG, (tag & 0xFF) + 1, 0)
        flags[s % slots] = raw
        extra(s, raw, arrived)
        return raw

    def unpack(s, side, inbox, slots, flags, release):
        ring, pos_ref = rings.at[side], state.at[side]

        def to_ring(rows, i):
            _word(ring, i)[...] = inbox[s % slots, rows]

        for_words(s, to_ring)

        @pl.loop(_blocks_decodable(s - 1), _blocks_decodable(s))
        def _(t):
            packet, raw, dst = inbox.at[t % slots], flags[t % slots], staging(side, t)
            free_staging(side, t)

            @pl.when(raw == 0)
            def _():
                pos_ref[...] = _decode(t, packet, ring, pos_ref[...], bases[side], dst)

            @pl.when(raw != 0)
            def _():
                for k in range(GROUPS):
                    low, high = _slab(packet, LOW_AT, k)[...], _slab(packet, HIGH_AT, k)[...]
                    _put_group(k, low, high, dst)
                bases[side] = raw - 1

            pos_ref[...] = _rebase(pos_ref[...], t)
            store(side, t, start)
            release(t)

    def relayed(t):
        whole(x_hop, t, y_raw[t % Y_SLOTS], sent)

    def release_y(t):
        @pl.when(t >= 1)
        def _():
            relayed(t - 1)
            give_credit(t - 1, Y_SLOTS, y_credit, y_peer)

    def release_x(t):
        give_credit(t, X_SLOTS, x_credit, x_peer)

    load(SHARED, 0)[0].start()
    barrier = pltpu.get_barrier_semaphore()
    for peer in (y_peer, x_peer):
        pl.semaphore_signal(barrier, 1, device_id=peer, device_id_type=mesh_id)
    rings[...] = jnp.zeros(rings.shape, jnp.int32)
    state[...] = jnp.zeros(state.shape, jnp.int32)
    for side in (SHARED, FROM_Y, FROM_X):
        bases[side] = jnp.int32(FIRST_BASE)

    @pl.loop(0, blocks + X_LAG)
    def _(s):
        r = s - Y_LAG
        relaying = (r >= 0) & (r < blocks)

        @pl.when(relaying)
        def _():
            y_head(r, arrived)
            take_credit(r, X_SLOTS, x_credit)
            x_head(r, start)

        first, last = (jnp.minimum(_blocks_encoded(i), blocks) for i in (s - 1, s))
        pl.loop(first, last)(encode)

        @pl.when(s < blocks)
        def _():
            def to_packet(rows, i):
                outbox[s % SEND_SLOTS, rows] = _word(rings.at[SHARED], i)[...]

            for_words(s, to_packet)

            @pl.when(s == 0)
            def _():
                pl.semaphore_wait(barrier, 2)

            take_credit(s, Y_SLOTS, y_credit)
            whole(y_hop, s, sent_raw[s % SEND_SLOTS], start)

        @pl.when(relaying)
        def _():
            raw = receive_tail(r, y_inbox, Y_SLOTS, y_raw, y_tail, y_extra)
            x_tail(r, start)
            x_extra(r, raw, start)
            unpack(r, FROM_Y, y_inbox, Y_SLOTS, y_raw, release_y)

        @pl.when(s >= X_LAG)
        def _():
            t = s - X_LAG
            x_head(t, arrived)
            receive_tail(t, x_inbox, X_SLOTS, x_raw, x_tail, x_extra)
            unpack(t, FROM_X, x_inbox, X_SLOTS, x_raw, release_x)

        t = s - PRIVATE_LAG

        @pl.when((t + 1 >= 0) & (t + 1 < blocks))
        def _():
            load(PRIVATE, t + 1)[0].start()

        @pl.when((t >= 0) & (t < blocks))
        def _():
            free_staging(PRIVATE, t)
            copy, src = load(PRIVATE, t)
            copy.wait()
            staging(PRIVATE, t)[...] = src[...].astype(jnp.bfloat16)
            store(PRIVATE, t, start)

    relayed(jnp.int32(blocks - 1))

    @pl.loop(blocks - SEND_SLOTS, blocks)
    def _(t):
        whole(y_hop, t, sent_raw[t % SEND_SLOTS], sent)

    @pl.loop(blocks - STORE_SLOTS, blocks)
    def _(t):
        for side in quarter:
            store(side, t, done)


def pallas_dist_ag_xy_y_m65536_n1024_kernel(x: jax.Array):
    rows, cols = x.shape
    run_rows = PIECES * PIECE_ROWS
    runs = rows // run_rows
    kept_rows = KEPT * PIECE_ROWS
    block = (RUNS, PIECE_ROWS, cols)
    dma = pltpu.SemaphoreType.DMA
    kept, spilled = pl.pallas_call(
        _kernel,
        out_shape=(
            pltpu.VMEM((2 * runs, kept_rows, cols), jnp.bfloat16),
            jax.ShapeDtypeStruct((2 * runs, run_rows - kept_rows, cols), jnp.bfloat16),
        ),
        in_specs=[pl.BlockSpec(memory_space=pl.ANY)],
        out_specs=(
            pl.BlockSpec(memory_space=pltpu.VMEM),
            pl.BlockSpec(memory_space=pl.ANY),
        ),
        scratch_shapes=[
            pltpu.VMEM((2 * LOAD_SLOTS, *block), jnp.float32),
            pltpu.VMEM((4 * STORE_SLOTS, *block), jnp.bfloat16),
            pltpu.VMEM((SEND_SLOTS, PACKET_ROWS, LANES), jnp.int32),
            pltpu.VMEM((Y_SLOTS, PACKET_ROWS, LANES), jnp.int32),
            pltpu.VMEM((X_SLOTS, PACKET_ROWS, LANES), jnp.int32),
            pltpu.VMEM((3, 8 * RING, LANES), jnp.int32),
            pltpu.VMEM((4, 8, LANES), jnp.int32),
            pltpu.SMEM((3,), jnp.int32),
            pltpu.SMEM((SEND_SLOTS,), jnp.int32),
            pltpu.SMEM((Y_SLOTS,), jnp.int32),
            pltpu.SMEM((X_SLOTS,), jnp.int32),
            dma((2 * LOAD_SLOTS,)),
            dma((4 * STORE_SLOTS,)),
            dma((3 * SEND_SLOTS,)),
            dma((3 * Y_SLOTS,)),
            dma((3 * Y_SLOTS,)),
            dma((3 * X_SLOTS,)),
            pltpu.SemaphoreType.REGULAR((2,)),
            pltpu.SemaphoreType.REGULAR((2,)),
        ],
        compiler_params=pltpu.CompilerParams(vmem_limit_bytes=16 * 2**20, collective_id=0),
    )(x.reshape(runs, run_rows, cols))

    def pieces(a, first, last):
        return a[:, first * PIECE_ROWS : last * PIECE_ROWS]

    parts = [
        pieces(kept, KEPT_SHIFT, KEPT),
        pieces(kept, 0, KEPT_SHIFT),
        lax.optimization_barrier(pieces(spilled, 0, 27)),
        lax.optimization_barrier(pieces(spilled, 27, 34)),
        pieces(spilled, 34, PIECES - KEPT),
    ]
    return jnp.concatenate(parts, axis=1).reshape(2 * rows, cols)
```
